```python
import numpy as np

kernel_name = "dist_ag_xy_y_m256_n256"

def setup_inputs():
    return {"x": np.random.randn(512, 256).astype(np.float32)}

def reference(x: np.ndarray) -> np.ndarray:
    return x
```

```python
import jax
import jax.numpy as jnp
from jax import lax
from jax.experimental import pallas as pl
from jax.experimental.pallas import tpu as pltpu

NCHUNK = 4


def pallas_dist_ag_xy_y_m256_n256_kernel(
x: jax.Array,
):
    m, n = x.shape
    c = m // NCHUNK
    MESH = pl.DeviceIdType.MESH

    def body(x_hbm, out_hbm, xv, sbuf, rbuf, ov, in_sems, loc_sem, send_sems,
             recv_sems, out_sems):
        my_x = lax.axis_index("x")
        my_y = lax.axis_index("y")
        peer = (my_x, 1 - my_y)

        barrier = pltpu.get_barrier_semaphore()
        pl.semaphore_signal(barrier, inc=1, device_id=peer, device_id_type=MESH)

        loads = []
        for k in range(NCHUNK):
            rows = pl.ds(k * c, c)
            cp = pltpu.make_async_copy(x_hbm.at[rows], xv.at[rows], in_sems.at[k])
            cp.start()
            loads.append(cp)
        local = pltpu.make_async_copy(
            x_hbm, out_hbm.at[pl.ds(pl.multiple_of(my_y * m, m), m)], loc_sem)
        local.start()

        for k in range(NCHUNK):
            rows = pl.ds(k * c, c)
            loads[k].wait()
            sbuf[rows, :] = xv[rows, :].astype(jnp.bfloat16)

        pl.semaphore_wait(barrier, 1)

        rdmas = []
        for k in range(NCHUNK):
            rows = pl.ds(k * c, c)
            r = pltpu.make_async_remote_copy(
                src_ref=sbuf.at[rows], dst_ref=rbuf.at[rows],
                send_sem=send_sems.at[k], recv_sem=recv_sems.at[k],
                device_id=peer, device_id_type=MESH)
            r.start()
            rdmas.append(r)

        stores = []
        base = pl.multiple_of((1 - my_y) * m, m)
        for k in range(NCHUNK):
            rows = pl.ds(k * c, c)
            rdmas[k].wait_recv()
            ov[rows, :] = rbuf[rows, :].astype(jnp.float32)
            st = pltpu.make_async_copy(
                ov.at[rows], out_hbm.at[pl.ds(base + k * c, c)], out_sems.at[k])
            st.start()
            stores.append(st)

        for k in range(NCHUNK):
            rdmas[k].wait_send()
        local.wait()
        for k in range(NCHUNK):
            stores[k].wait()

    return pl.pallas_call(
        body,
        out_shape=jax.ShapeDtypeStruct((2 * m, n), x.dtype),
        in_specs=[pl.BlockSpec(memory_space=pl.ANY)],
        out_specs=pl.BlockSpec(memory_space=pl.ANY),
        scratch_shapes=[
            pltpu.VMEM((m, n), x.dtype),
            pltpu.VMEM((m, n), jnp.bfloat16),
            pltpu.VMEM((m, n), jnp.bfloat16),
            pltpu.VMEM((m, n), x.dtype),
            pltpu.SemaphoreType.DMA((NCHUNK,)),
            pltpu.SemaphoreType.DMA,
            pltpu.SemaphoreType.DMA((NCHUNK,)),
            pltpu.SemaphoreType.DMA((NCHUNK,)),
            pltpu.SemaphoreType.DMA((NCHUNK,)),
        ],
        compiler_params=pltpu.CompilerParams(collective_id=0),
    )(x)
```

```python
import jax
import jax.numpy as jnp
from jax import lax
from jax.experimental import pallas as pl
from jax.experimental.pallas import tpu as pltpu

HEAD = 16
CHUNKS = (32, 176, 32)


def pallas_dist_ag_xy_y_m256_n256_kernel(
x: jax.Array,
):
    m, n = x.shape
    assert HEAD + sum(CHUNKS) == m
    nc = len(CHUNKS)
    starts = [HEAD + sum(CHUNKS[:k]) for k in range(nc)]
    MESH = pl.DeviceIdType.MESH

    def body(x_hbm, out_ref, sbuf, rbuf, in_sems, send_sems, recv_sems):
        my_y = lax.axis_index("y")
        peer = (lax.axis_index("x"), 1 - my_y)

        barrier = pltpu.get_barrier_semaphore()
        pl.semaphore_signal(barrier, inc=1, device_id=peer, device_id_type=MESH)

        def mine(start, size):
            return pl.ds(pl.multiple_of(my_y * m + start, 16), size)

        def theirs(start, size):
            return pl.ds(pl.multiple_of((1 - my_y) * m + start, 16), size)

        loads = []
        for k in range(nc):
            lo = 0 if k == 0 else starts[k]
            size = starts[k] + CHUNKS[k] - lo
            cp = pltpu.make_async_copy(
                x_hbm.at[pl.ds(lo, size)], out_ref.at[mine(lo, size)], in_sems.at[k])
            cp.start()
            loads.append(cp)
        if HEAD:
            pl.semaphore_wait(barrier, 1)
            head = pltpu.make_async_remote_copy(
                src_ref=x_hbm.at[pl.ds(0, HEAD)], dst_ref=out_ref.at[mine(0, HEAD)],
                send_sem=send_sems.at[nc], recv_sem=recv_sems.at[nc],
                device_id=peer, device_id_type=MESH)
            head.start()

        rdmas = []
        for k in range(nc):
            rows = pl.ds(starts[k], CHUNKS[k])
            loads[k].wait()
            sbuf[rows, :] = out_ref[mine(starts[k], CHUNKS[k]), :].astype(jnp.bfloat16)
            if k == 0 and not HEAD:
                pl.semaphore_wait(barrier, 1)
            r = pltpu.make_async_remote_copy(
                src_ref=sbuf.at[rows], dst_ref=rbuf.at[rows],
                send_sem=send_sems.at[k], recv_sem=recv_sems.at[k],
                device_id=peer, device_id_type=MESH)
            r.start()
            rdmas.append(r)

        if HEAD:
            head.wait()
        for k in range(nc):
            rows = pl.ds(starts[k], CHUNKS[k])
            rdmas[k].wait_recv()
            out_ref[theirs(starts[k], CHUNKS[k]), :] = rbuf[rows, :].astype(out_ref.dtype)
        for k in range(nc):
            rdmas[k].wait_send()

    return pl.pallas_call(
        body,
        out_shape=jax.ShapeDtypeStruct((2 * m, n), x.dtype),
        in_specs=[pl.BlockSpec(memory_space=pltpu.HBM)],
        out_specs=pl.BlockSpec(memory_space=pltpu.VMEM),
        scratch_shapes=[
            pltpu.VMEM((m, n), jnp.bfloat16),
            pltpu.VMEM((m, n), jnp.bfloat16),
            pltpu.SemaphoreType.DMA((nc,)),
            pltpu.SemaphoreType.DMA((nc + 1,)),
            pltpu.SemaphoreType.DMA((nc + 1,)),
        ],
        compiler_params=pltpu.CompilerParams(collective_id=0),
    )(x)
```
